```python
import numpy as np

kernel_name = "dist_ring_attn_i_s256_d64"

def setup_inputs():
    S, D = 1024, 64
    q = np.random.randn(S, D).astype(np.float32)
    k = np.random.randn(S, D).astype(np.float32)
    v = np.random.randn(S, D).astype(np.float32)
    return {"q": q, "k": k, "v": v}

def reference(q: np.ndarray, k: np.ndarray, v: np.ndarray) -> np.ndarray:
    D = q.shape[1]
    scores = q @ k.T / np.sqrt(D)
    scores_max = np.max(scores, axis=1, keepdims=True)
    weights = np.exp(scores - scores_max)
    weights = weights / np.sum(weights, axis=1, keepdims=True)
    return weights @ v
```

```python
import jax
import jax.numpy as jnp
from jax import lax
from jax.experimental import pallas as pl
from jax.experimental.pallas import tpu as pltpu

N_DEV = 4
LOG2E = 1.4426950408889634


def pallas_dist_ring_attn_i_s256_d64_kernel(q: jax.Array, k: jax.Array, v: jax.Array):
    def body(q_hbm, k_hbm, v_hbm, o_ref, q32, k32, v32, kv, qab, lsem, ssem, rsem):
        me = lax.axis_index("i")
        right = (me + 1) % N_DEV
        left = (me + 3) % N_DEV
        diag = (me + 2) % N_DEV
        bs = pltpu.get_barrier_semaphore()
        for t in (right, left, diag):
            pl.semaphore_signal(bs, inc=1, device_id=(t,), device_id_type=pl.DeviceIdType.MESH)
        ck = pltpu.make_async_copy(k_hbm, k32, lsem.at[0])
        ck.start()
        cv = pltpu.make_async_copy(v_hbm, v32, lsem.at[1])
        cv.start()
        cq = pltpu.make_async_copy(q_hbm, q32, lsem.at[2])
        cq.start()
        ck.wait()
        kt = k32[...]
        kab = jnp.concatenate([kt[:, :128], kt[:, 128:]], axis=0)
        kv[0, 0:128, :] = kab.T.astype(jnp.bfloat16)
        cv.wait()
        vt = v32[...].astype(jnp.bfloat16)
        kv[0, 128:192, :] = vt[:, :128]
        kv[0, 192:256, :] = vt[:, 128:]
        pl.semaphore_wait(bs, 3)
        cps = []
        for s, d in ((1, right), (2, left), (3, diag)):
            cp = pltpu.make_async_remote_copy(
                kv.at[0], kv.at[s], ssem.at[s], rsem.at[s],
                device_id=(d,), device_id_type=pl.DeviceIdType.MESH)
            cp.start()
            cps.append(cp)
        cq.wait()
        qt = (q32[...] * (LOG2E / 8.0)).astype(jnp.bfloat16)
        z = jnp.zeros_like(qt)
        qab[...] = jnp.concatenate(
            [jnp.concatenate([qt, z], 0), jnp.concatenate([z, qt], 0)], 1)

        def block(j, m, l, acc):
            x = kv[j, 0:128, :]
            s = jnp.dot(x, qab[...], preferred_element_type=jnp.float32)
            mb = jnp.max(s, axis=0, keepdims=True)
            mb = jnp.maximum(mb[:, :256], mb[:, 256:])
            mn = mb if m is None else jnp.maximum(m, mb)
            m2 = jnp.concatenate([mn, mn], axis=1)
            p = jnp.exp2(s - m2)
            ls = jnp.sum(p, axis=0, keepdims=True)
            ls = ls[:, :256] + ls[:, 256:]
            pb = p.astype(jnp.bfloat16)
            pc = jnp.concatenate([pb[:, :256], pb[:, 256:]], axis=0)
            vtj = jnp.concatenate([kv[j, 128:192, :], kv[j, 192:256, :]], axis=1)
            pv = jnp.dot(vtj, pc, preferred_element_type=jnp.float32)
            if m is None:
                return mn, ls, pv
            alpha = jnp.exp2(m - mn)
            return mn, alpha * l + ls, alpha * acc + pv

        m, l, acc = block(0, None, None, None)
        for s in (1, 2, 3):
            cps[s - 1].wait_recv()
            m, l, acc = block(s, m, l, acc)
        o_ref[...] = acc / l
        for cp in cps:
            cp.wait_send()

    o = pl.pallas_call(
        body,
        out_shape=jax.ShapeDtypeStruct((64, 256), q.dtype),
        in_specs=[pl.BlockSpec(memory_space=pl.ANY)] * 3,
        out_specs=pl.BlockSpec(memory_space=pltpu.VMEM),
        scratch_shapes=[pltpu.VMEM((64, 256), jnp.float32)] * 3 + [
            pltpu.VMEM((4, 256, 128), jnp.bfloat16),
            pltpu.VMEM((128, 512), jnp.bfloat16),
            pltpu.SemaphoreType.DMA((3,)),
            pltpu.SemaphoreType.DMA((4,)),
            pltpu.SemaphoreType.DMA((4,)),
        ],
        compiler_params=pltpu.CompilerParams(collective_id=0),
    )(q.T, k.T, v.T)
    return o.T
```

```python
import jax
import jax.numpy as jnp
from jax import lax
from jax.experimental import pallas as pl
from jax.experimental.pallas import tpu as pltpu

_SCALE = 1.4426950408889634 / 8.0
_MESH = pl.DeviceIdType.MESH
_K, _KA, _KB = (0, 128), (0, 64), (64, 64)
_V, _VA, _VB = (128, 128), (128, 64), (192, 64)
_OWN, _A, _B, _C = 0, 1, 2, 3

_SENDS = {
    0: dict(k01=(_OWN, _K, 1, _A, "k"), k03=(_OWN, _K, 3, _A, "k"),
            v01=(_OWN, _V, 1, _A, "v"), v03=(_OWN, _V, 3, _A, "v"),
            k02=(_OWN, _K, 2, _B, "k"), v02=(_OWN, _V, 2, _B, "v"),
            k31=(_A, _K, 1, _C, "k"), v31=(_A, _V, 1, _C, "v")),
    1: dict(k10a=(_OWN, _KA, 0, _B, "k"), k10b=(_OWN, _KB, 0, _B, "k"), v10=(_OWN, _V, 0, _B, "v"),
            k13=(_OWN, _K, 3, _C, "k"), v13=(_OWN, _V, 3, _C, "v"),
            k12=(_OWN, _K, 2, _C, "k"), v12=(_OWN, _V, 2, _C, "v")),
    2: dict(b23=(_OWN, _VB, 3, _B, "x"), k20=(_OWN, _K, 0, _C, "k"), a20=(_OWN, _VA, 0, _C, "v"),
            k23=(_OWN, _K, 3, _B, "k"), a23=(_OWN, _VA, 3, _B, "v"),
            k21=(_OWN, _K, 1, _B, "k"), v21=(_OWN, _V, 1, _B, "v")),
    3: dict(k30=(_OWN, _K, 0, _A, "k"), v30=(_OWN, _V, 0, _A, "v"),
            k32=(_OWN, _K, 2, _A, "k"), v32=(_OWN, _V, 2, _A, "v"),
            f30=(_B, _VB, 0, _C, "x")),
}


def _attention_kernel(q_hbm, k_hbm, v_hbm, o_ref, q32, k32, v32, kv, qs, pbuf, accb,
                      lsem, ssem, rk, rv, rx, esem):
    me = lax.axis_index("i")
    barrier = pltpu.get_barrier_semaphore()
    bf16 = jnp.bfloat16
    f32 = jnp.float32

    def lanes(ref, half):
        return ref.at[:, pl.ds(128 * half, 128)]

    load_k = pltpu.make_async_copy(k_hbm, k32, lsem.at[0])
    load_v = pltpu.make_async_copy(v_hbm, v32, lsem.at[1])
    load_q = pltpu.make_async_copy(q_hbm, q32, lsem.at[2])

    def load_half(hbm, vmem, half, sem):
        return pltpu.make_async_copy(lanes(hbm, half), lanes(vmem, half), lsem.at[sem])

    def recv_sem(slot, kind):
        return {"k": rk, "v": rv}[kind].at[slot - 1] if kind != "x" else rx

    def remote(src_slot, rows, target, dst_slot, kind):
        return pltpu.make_async_remote_copy(
            kv.at[src_slot, pl.ds(*rows)], kv.at[dst_slot, pl.ds(*rows)], ssem,
            recv_sem(dst_slot, kind), device_id=(target,), device_id_type=_MESH)

    def send(role, *names):
        for name in names:
            remote(*_SENDS[role][name]).start()

    def recv(slot, rows, kind):
        remote(_OWN, rows, 0, slot, kind).wait_recv()

    def signal(sem, *targets):
        for target in targets:
            pl.semaphore_signal(sem, inc=1, device_id=(target,), device_id_type=_MESH)

    def cast(src32, half, row):
        kv[_OWN, row:row + 64, :] = src32[:, 128 * half:128 * (half + 1)].astype(bf16)

    def cast_k():
        load_k.wait()
        cast(k32, 0, 0)
        cast(k32, 1, 64)

    def cast_v():
        load_v.wait()
        cast(v32, 0, 128)
        cast(v32, 1, 192)

    @pl.when(me == 1)
    def _():
        load_ka, load_kb = load_half(k_hbm, k32, 0, 0), load_half(k_hbm, k32, 1, 3)
        load_ka.start(); load_kb.start(); load_v.start(); load_q.start()
        signal(barrier, 0, 2)
        pl.semaphore_wait(barrier, 1)
        load_ka.wait()
        cast(k32, 0, 0)
        send(1, "k10a")
        load_kb.wait()
        cast(k32, 1, 64)
        send(1, "k10b")
        cast_v()
        send(1, "v10")

    @pl.when(me == 2)
    def _():
        load_va, load_vb = load_half(v_hbm, v32, 0, 1), load_half(v_hbm, v32, 1, 3)
        load_vb.start(); load_k.start(); load_va.start(); load_q.start()
        pl.semaphore_wait(barrier, 3)
        signal(esem, 1, 3, 0)
        load_vb.wait()
        cast(v32, 1, 192)
        send(2, "b23")
        cast_k()
        send(2, "k20")
        load_va.wait()
        cast(v32, 0, 128)
        send(2, "a20", "k23", "a23", "k21", "v21")

    @pl.when(me == 3)
    def _():
        load_k.start(); load_v.start(); load_q.start()
        signal(barrier, 0, 2)
        pl.semaphore_wait(barrier, 1)
        cast_k()
        send(3, "k30")
        cast_v()
        send(3, "v30")

    @pl.when(me == 0)
    def _():
        load_k.start(); load_v.start(); load_q.start()
        signal(barrier, 1, 3, 2)
        cast_k()
        cast_v()
        pl.semaphore_wait(barrier, 2)
        send(0, "k01", "k03", "v01", "v03")

    load_q.wait()
    qt = (q32[...] * _SCALE).astype(bf16)
    qs[0] = qt[:, :128]
    qs[1] = qt[:, 128:]

    def scores(slot, m_run):
        k = [kv[slot, 64 * kh:64 * (kh + 1), :].T for kh in range(2)]
        ms, alphas, sums = [], [], []
        for h in range(2):
            s = [jnp.dot(k[kh], qs[h], preferred_element_type=f32) for kh in range(2)]
            m = jnp.max(jnp.maximum(s[0], s[1]), axis=0, keepdims=True)
            if m_run is not None:
                m_old, m = m_run[h], jnp.maximum(m_run[h], m)
                alphas.append(jnp.exp2(m_old - m))
            p = [jnp.exp2(x - m) for x in s]
            for kh in range(2):
                pbuf[slot, h, 128 * kh:128 * (kh + 1), :] = p[kh].astype(bf16)
            part = p[0] + p[1]
            part = [part[8 * i:8 * (i + 1)] for i in range(16)]
            while len(part) > 1:
                part = [part[i] + part[i + 1] for i in range(0, len(part), 2)]
            ms.append(m)
            sums.append(part[0])
        return ms, alphas, sums

    def rowsum(part):
        return jnp.sum(part, axis=0, keepdims=True)

    def pv(slot):
        va, vb = kv[slot, 128:192, :], kv[slot, 192:256, :]
        return [jnp.dot(va, pbuf[slot, h, 0:128, :], preferred_element_type=f32)
                + jnp.dot(vb, pbuf[slot, h, 128:256, :], preferred_element_type=f32)
                for h in range(2)]

    m, _, sums = scores(_OWN, None)
    l = [rowsum(x) for x in sums]
    acc = pv(_OWN)

    @pl.when(me == 0)
    def _():
        pl.semaphore_wait(esem, 1)
        send(0, "k02", "v02")

    @pl.when(me == 1)
    def _():
        pl.semaphore_wait(esem, 1)
        send(1, "k13", "v13", "k12", "v12")

    @pl.when(me == 3)
    def _():
        pl.semaphore_wait(esem, 1)
        send(3, "k32", "v32")
        recv(_B, _VB, "x")
        send(3, "f30")

    recv(_A, _K, "k")

    @pl.when(me == 0)
    def _():
        send(0, "k31")

    m, al_a, sums = scores(_A, m)
    l = [l[h] * al_a[h] + rowsum(sums[h]) for h in range(2)]

    @pl.when(me != 0)
    def _():
        recv(_A, _V, "v")
        pa = pv(_A)
        for h in range(2):
            accb[h] = acc[h] * al_a[h] + pa[h]

    recv(_B, _K, "k")
    m, al_b, sums = scores(_B, m)
    l = [l[h] * al_b[h] + rowsum(sums[h]) for h in range(2)]

    @pl.when(me == 0)
    def _():
        recv(_A, _V, "v")
        send(0, "v31")
        pa = pv(_A)
        acc_a = [acc[h] * al_a[h] + pa[h] for h in range(2)]
        recv(_B, _V, "v")
        pb = pv(_B)
        for h in range(2):
            accb[h] = acc_a[h] * al_b[h] + pb[h]

    recv(_C, _K, "k")
    m, al_c, sums = scores(_C, m)

    @pl.when(me != 0)
    def _():
        @pl.when(me == 3)
        def _():
            recv(_B, _VA, "v")

        @pl.when(me != 3)
        def _():
            recv(_B, _V, "v")

        pb = pv(_B)
        for h in range(2):
            accb[h] = accb[h] * al_b[h] + pb[h]

    @pl.when(me == 0)
    def _():
        recv(_C, _VA, "v")
        recv(_C, _VB, "x")

    @pl.when(me != 0)
    def _():
        recv(_C, _V, "v")

    pc = pv(_C)
    for h in range(2):
        inv_l = 1.0 / (l[h] * al_c[h] + rowsum(sums[h]))
        o_ref[:, 128 * h:128 * (h + 1)] = accb[h] * (al_c[h] * inv_l) + pc[h] * inv_l

    for role, sends in _SENDS.items():
        slots, rest = divmod(sum(s[1][1] for s in sends.values()), 256)

        @pl.when(me == role)
        def _(slots=slots, rest=rest):
            whole = kv.at[pl.ds(0, slots)]
            pltpu.make_async_copy(whole, whole, ssem).wait()
            if rest:
                part = kv.at[3, pl.ds(0, rest)]
                pltpu.make_async_copy(part, part, ssem).wait()


def pallas_dist_ring_attn_i_s256_d64_kernel(q: jax.Array, k: jax.Array, v: jax.Array):
    s, d = q.shape
    o_t = pl.pallas_call(
        _attention_kernel,
        out_shape=jax.ShapeDtypeStruct((d, s), q.dtype),
        in_specs=[pl.BlockSpec(memory_space=pl.ANY)] * 3,
        out_specs=pl.BlockSpec(memory_space=pltpu.VMEM),
        scratch_shapes=[
            pltpu.VMEM((d, s), jnp.float32),
            pltpu.VMEM((d, s), jnp.float32),
            pltpu.VMEM((d, s), jnp.float32),
            pltpu.VMEM((4, 256, 128), jnp.bfloat16),
            pltpu.VMEM((2, d, 128), jnp.bfloat16),
            pltpu.VMEM((4, 2, 256, 128), jnp.bfloat16),
            pltpu.VMEM((2, d, 128), jnp.float32),
            pltpu.SemaphoreType.DMA((4,)),
            pltpu.SemaphoreType.DMA,
            pltpu.SemaphoreType.DMA((3,)),
            pltpu.SemaphoreType.DMA((3,)),
            pltpu.SemaphoreType.DMA,
            pltpu.SemaphoreType.REGULAR,
        ],
        compiler_params=pltpu.CompilerParams(collective_id=0, disable_semaphore_checks=True),
    )(q.T, k.T, v.T)
    return o_t.T
```
